```python
import numpy as np

kernel_name = "dist_mean_ax1_xy_m1024_n512"

def setup_inputs():
    return {"x": np.random.randn(2048, 1024).astype(np.float32)}

def reference(x: np.ndarray) -> np.ndarray:
    return np.mean(x, axis=1, keepdims=True)
```

```python
import jax
import jax.numpy as jnp
from jax import lax
from jax.experimental import pallas as pl
from jax.experimental.pallas import tpu as pltpu

LANES = 128


def _block_row_sums(buf, r0):
    n = buf.shape[1]
    xs = buf[pl.ds(r0, LANES), :]
    p = xs[:, 0:LANES]
    for c in range(LANES, n, LANES):
        p = p + xs[:, c:c + LANES]
    s = jnp.sum(p, axis=1, keepdims=True)
    ri = lax.broadcasted_iota(jnp.int32, (LANES, LANES), 0)
    li = lax.broadcasted_iota(jnp.int32, (LANES, LANES), 1)
    return jnp.sum(jnp.where(ri == li, s, 0.0), axis=0, keepdims=True)


def pallas_dist_mean_ax1_xy_m1024_n512_kernel(x: jax.Array):
    m, n = x.shape
    scale = 1.0 / (2 * n)
    chunks = [(0, m - LANES), (m - LANES, LANES)]

    def body(x_hbm, out_ref, buf, part, recv, load_sems, send_sems, recv_sems):
        peer = (lax.axis_index("x"), 1 - lax.axis_index("y"))
        loads = [
            pltpu.make_async_copy(
                x_hbm.at[pl.ds(s, c)], buf.at[pl.ds(s, c)], load_sems.at[i])
            for i, (s, c) in enumerate(chunks)
        ]
        for cp in loads:
            cp.start()

        barrier = pltpu.get_barrier_semaphore()
        pl.semaphore_signal(barrier, inc=1, device_id=peer,
                            device_id_type=pl.DeviceIdType.MESH)
        pl.semaphore_wait(barrier, 1)

        rdmas = []
        for i, (s, c) in enumerate(chunks):
            loads[i].wait()
            for r in range(s, s + c, LANES):
                part[:, pl.ds(r, LANES)] = _block_row_sums(buf, r)
            rdma = pltpu.make_async_remote_copy(
                src_ref=part.at[:, pl.ds(s, c)], dst_ref=recv.at[:, pl.ds(s, c)],
                send_sem=send_sems.at[i], recv_sem=recv_sems.at[i],
                device_id=peer, device_id_type=pl.DeviceIdType.MESH)
            rdma.start()
            rdmas.append(rdma)
        for rdma, (s, c) in zip(rdmas, chunks):
            rdma.wait_recv()
            out_ref[:, pl.ds(s, c)] = (
                part[:, pl.ds(s, c)] + recv[:, pl.ds(s, c)]) * scale
        for rdma in rdmas:
            rdma.wait_send()

    out = pl.pallas_call(
        body,
        out_shape=jax.ShapeDtypeStruct((1, m), jnp.float32),
        in_specs=[pl.BlockSpec(memory_space=pl.ANY)],
        out_specs=pl.BlockSpec(memory_space=pltpu.VMEM),
        scratch_shapes=[
            pltpu.VMEM((m, n), jnp.float32),
            pltpu.VMEM((1, m), jnp.float32),
            pltpu.VMEM((1, m), jnp.float32),
            pltpu.SemaphoreType.DMA((len(chunks),)),
            pltpu.SemaphoreType.DMA((len(chunks),)),
            pltpu.SemaphoreType.DMA((len(chunks),)),
        ],
        compiler_params=pltpu.CompilerParams(
            collective_id=0,
            disable_semaphore_checks=True,
            disable_bounds_checks=True,
        ),
    )(x)
    return out.reshape(m, 1)
```

```python
import jax
import jax.numpy as jnp
from jax import lax
from jax.experimental import pallas as pl
from jax.experimental.pallas import tpu as pltpu

LANES = 128
SUBLANES = 8
MESH = pl.DeviceIdType.MESH

M = 1024
LAST = M - LANES
RAW = 56
RAW0 = LAST - RAW
RAW_BLK = RAW0 // LANES * LANES

FIRST = (0, 512)
EARLY_CHUNKS = (FIRST, (LAST, LANES), (512, LAST - 512))
LATE_CHUNKS = (FIRST, (512, RAW0 - LANES - 512), (RAW0 - LANES, LANES),
               (LAST, 64), (LAST + 64, 64), (RAW0, RAW))


def _scatter_row_sums(ref, r0, rows, lane0):
    xs = ref[pl.ds(r0, rows), :]
    tiles = [xs[:, c:c + LANES] for c in range(0, xs.shape[1], LANES)]
    while len(tiles) > 1:
        tiles = [tiles[i] + tiles[i + 1] for i in range(0, len(tiles), 2)]
    s = jnp.sum(tiles[0], axis=1, keepdims=True)
    row = lax.broadcasted_iota(jnp.int32, (rows, LANES), 0) + lane0
    lane = lax.broadcasted_iota(jnp.int32, (rows, LANES), 1)
    w = jnp.where(row == lane, s, 0.0)
    acc = w[0:SUBLANES]
    for g in range(SUBLANES, rows, SUBLANES):
        acc = acc + w[g:g + SUBLANES]
    return acc


def _squash(acc):
    return jnp.sum(acc, axis=0, keepdims=True)


def _compiler_params():
    try:
        return pltpu.CompilerParams(collective_id=0,
                                    disable_bounds_checks=True,
                                    disable_semaphore_checks=True)
    except TypeError:
        return pltpu.CompilerParams(collective_id=0)


def pallas_dist_mean_ax1_xy_m1024_n512_kernel(x: jax.Array):
    m, n = x.shape
    assert m == M and n == 4 * LANES
    scale = 1.0 / (2 * n)

    def body(x_hbm, out_ref, buf, rawbuf, part, recv,
             load_sems, send_sems, recv_sems):
        def load(i, chunk):
            rows = pl.ds(*chunk)
            return pltpu.make_async_copy(
                x_hbm.at[rows], buf.at[rows], load_sems.at[i])

        load(0, FIRST).start()

        my_y = lax.axis_index("y")
        peer = (lax.axis_index("x"), 1 - my_y)
        barrier = pltpu.get_barrier_semaphore()

        def remote(k, src, dst):
            return pltpu.make_async_remote_copy(
                src_ref=src, dst_ref=dst,
                send_sem=send_sems.at[k], recv_sem=recv_sems.at[k],
                device_id=peer, device_id_type=MESH)

        head = pl.ds(0, LAST)
        last = pl.ds(LAST, LANES)
        msg_head = lambda: remote(0, part.at[:, head], recv.at[:, head])
        msg_last_part = lambda: remote(1, part.at[:, last], recv.at[:, last])
        msg_last_out = lambda: remote(1, out_ref.at[:, last], out_ref.at[:, last])
        msg_raw = lambda: remote(2, x_hbm.at[pl.ds(RAW0, RAW)], rawbuf)

        def reduce_chunk(chunk, acc, stop):
            r, end = chunk[0], chunk[0] + chunk[1]
            while r < end:
                rows = min(end - r, LANES - r % LANES)
                c = _scatter_row_sums(buf, r, rows, r % LANES)
                acc = c if acc is None else acc + c
                blk = r // LANES * LANES
                r += rows
                if r % LANES == 0 or r == stop:
                    part[:, pl.ds(blk, LANES)] = _squash(acc)
                    acc = None
            return acc

        def finish_head(raw_sums):
            lo = pl.ds(0, RAW_BLK)
            out_ref[:, lo] = (part[:, lo] + recv[:, lo]) * scale
            hi = pl.ds(RAW_BLK, LANES)
            out_ref[:, hi] = (part[:, hi] + recv[:, hi] + raw_sums) * scale

        @pl.when(my_y == 0)
        def _():
            for i in range(1, len(EARLY_CHUNKS)):
                load(i, EARLY_CHUNKS[i]).start()
            pl.semaphore_signal(barrier, inc=1, device_id=peer,
                                device_id_type=MESH)
            for i in range(2):
                load(i, EARLY_CHUNKS[i]).wait()
                reduce_chunk(EARLY_CHUNKS[i], None, None)
            pl.semaphore_wait(barrier, 1)
            msg_last_part().start()
            load(2, EARLY_CHUNKS[2]).wait()
            reduce_chunk(EARLY_CHUNKS[2], None, None)
            msg_head().start()

            msg_raw().wait_recv()
            raw_sums = _squash(_scatter_row_sums(rawbuf, 0, RAW, RAW0 % LANES))
            msg_head().wait_recv()
            finish_head(raw_sums)
            msg_head().wait_send()
            msg_last_part().wait_send()
            msg_last_out().wait_recv()

        @pl.when(my_y == 1)
        def _():
            for i in range(1, len(LATE_CHUNKS)):
                load(i, LATE_CHUNKS[i]).start()
            pl.semaphore_signal(barrier, inc=1, device_id=peer,
                                device_id_type=MESH)
            pl.semaphore_wait(barrier, 1)
            msg_raw().start()

            acc = None
            for i in range(3):
                load(i, LATE_CHUNKS[i]).wait()
                acc = reduce_chunk(LATE_CHUNKS[i], acc, RAW0)
            msg_head().start()

            msg_last_part().wait_recv()
            sub = lax.broadcasted_iota(jnp.int32, (SUBLANES, LANES), 0)
            acc = jnp.where(sub == 0, recv[:, last], 0.0)
            for i in (3, 4):
                r0, rows = LATE_CHUNKS[i]
                load(i, LATE_CHUNKS[i]).wait()
                acc = acc + _scatter_row_sums(buf, r0, rows, r0 % LANES)
            out_ref[:, last] = _squash(acc) * scale
            msg_last_out().start()

            load(5, LATE_CHUNKS[5]).wait()
            raw_sums = _squash(_scatter_row_sums(buf, RAW0, RAW, RAW0 % LANES))
            msg_head().wait_recv()
            finish_head(raw_sums)
            msg_head().wait_send()
            msg_last_out().wait_send()
            msg_raw().wait_send()

    out = pl.pallas_call(
        body,
        out_shape=jax.ShapeDtypeStruct((1, m), jnp.float32),
        in_specs=[pl.BlockSpec(memory_space=pl.ANY)],
        out_specs=pl.BlockSpec(memory_space=pltpu.VMEM),
        scratch_shapes=[
            pltpu.VMEM((m, n), jnp.float32),
            pltpu.VMEM((RAW, n), jnp.float32),
            pltpu.VMEM((1, m), jnp.float32),
            pltpu.VMEM((1, m), jnp.float32),
            pltpu.SemaphoreType.DMA((len(LATE_CHUNKS),)),
            pltpu.SemaphoreType.DMA((3,)),
            pltpu.SemaphoreType.DMA((3,)),
        ],
        compiler_params=_compiler_params(),
    )(x)
    return out.reshape(m, 1)
```

```python
import jax
import jax.numpy as jnp
from jax import lax
from jax.experimental import pallas as pl
from jax.experimental.pallas import tpu as pltpu

LANES = 128
SUBLANES = 8
MESH = pl.DeviceIdType.MESH

M = 1024
LAST = M - LANES
MID = LAST - LANES
RAW = 56
RAW0 = LAST - RAW

FIRST = (0, 512)
EARLY_CHUNKS = (FIRST, (LAST, LANES), (512, MID - 512), (MID, LANES))
LATE_CHUNKS = (FIRST, (512, RAW0 - LANES - 512), (RAW0 - LANES, LANES),
               (LAST, 64), (LAST + 64, 64), (RAW0, RAW))


def _scatter_row_sums(ref, r0, rows, lane0, acc=None):
    xs = ref[pl.ds(r0, rows), :]
    tiles = [xs[:, c:c + LANES] for c in range(0, xs.shape[1], LANES)]
    while len(tiles) > 1:
        tiles = [tiles[i] + tiles[i + 1] for i in range(0, len(tiles), 2)]
    sums = jnp.sum(tiles[0], axis=1, keepdims=True)
    diag = (lax.broadcasted_iota(jnp.int32, (SUBLANES, LANES), 1)
            - lax.broadcasted_iota(jnp.int32, (SUBLANES, LANES), 0))
    if acc is None:
        acc = jnp.zeros((SUBLANES, LANES), jnp.float32)
    for g in range(0, rows, SUBLANES):
        acc = jnp.where(diag == lane0 + g, sums[g:g + SUBLANES], acc)
    return acc


def _squash(acc):
    return jnp.sum(acc, axis=0, keepdims=True)


def _compiler_params():
    try:
        return pltpu.CompilerParams(collective_id=0,
                                    disable_bounds_checks=True,
                                    disable_semaphore_checks=True)
    except TypeError:
        return pltpu.CompilerParams(collective_id=0)


def pallas_dist_mean_ax1_xy_m1024_n512_kernel(x: jax.Array):
    m, n = x.shape
    assert m == M and n == 4 * LANES
    scale = 1.0 / (2 * n)

    def body(x_hbm, out_ref, buf, rawbuf, part, recv,
             load_sems, send_sems, recv_sems):
        def load(i, chunk):
            rows = pl.ds(*chunk)
            return pltpu.make_async_copy(
                x_hbm.at[rows], buf.at[rows], load_sems.at[i])

        load(0, FIRST).start()

        my_y = lax.axis_index("y")
        peer = (lax.axis_index("x"), 1 - my_y)
        barrier = pltpu.get_barrier_semaphore()

        def remote(k, src, dst):
            return pltpu.make_async_remote_copy(
                src_ref=src, dst_ref=dst,
                send_sem=send_sems.at[k], recv_sem=recv_sems.at[k],
                device_id=peer, device_id_type=MESH)

        lo, mid, last = pl.ds(0, MID), pl.ds(MID, LANES), pl.ds(LAST, LANES)
        head = pl.ds(0, LAST)
        up_lo = lambda: remote(0, part.at[:, lo], recv.at[:, lo])
        up_last = lambda: remote(1, part.at[:, last], recv.at[:, last])
        up_mid = lambda: remote(2, part.at[:, mid], recv.at[:, mid])
        down_head = lambda: remote(0, part.at[:, head], recv.at[:, head])
        down_last = lambda: remote(1, out_ref.at[:, last], out_ref.at[:, last])
        down_raw = lambda: remote(2, x_hbm.at[pl.ds(RAW0, RAW)], rawbuf)

        def reduce_chunk(chunk, acc=None, stop=None):
            r, end = chunk[0], chunk[0] + chunk[1]
            while r < end:
                rows = min(end - r, LANES - r % LANES)
                acc = _scatter_row_sums(buf, r, rows, r % LANES, acc)
                blk = r // LANES * LANES
                r += rows
                if r % LANES == 0 or r == stop:
                    part[:, pl.ds(blk, LANES)] = _squash(acc)
                    acc = None
            return acc

        @pl.when(my_y == 1)
        def _():
            for i in range(1, len(LATE_CHUNKS)):
                load(i, LATE_CHUNKS[i]).start()
            pl.semaphore_signal(barrier, inc=1, device_id=peer,
                                device_id_type=MESH)
            pl.semaphore_wait(barrier, 1)
            down_raw().start()

            acc = None
            for i in range(3):
                load(i, LATE_CHUNKS[i]).wait()
                acc = reduce_chunk(LATE_CHUNKS[i], acc, RAW0)
            down_head().start()

            up_last().wait_recv()
            sub = lax.broadcasted_iota(jnp.int32, (SUBLANES, LANES), 0)
            lane = lax.broadcasted_iota(jnp.int32, (SUBLANES, LANES), 1)
            acc = jnp.where(sub == (lane + 1) % SUBLANES, recv[:, last], 0.0)
            for i in (3, 4):
                r0, rows = LATE_CHUNKS[i]
                load(i, LATE_CHUNKS[i]).wait()
                acc = _scatter_row_sums(buf, r0, rows, r0 % LANES, acc)
            out_ref[:, last] = _squash(acc) * scale
            down_last().start()

            load(5, LATE_CHUNKS[5]).wait()
            own_mid = part[:, mid] + _squash(
                _scatter_row_sums(buf, RAW0, RAW, RAW0 % LANES))
            down_raw().wait_send()
            down_head().wait_send()
            down_last().wait_send()
            up_lo().wait_recv()
            out_ref[:, lo] = (part[:, lo] + recv[:, lo]) * scale
            up_mid().wait_recv()
            out_ref[:, mid] = (own_mid + recv[:, mid]) * scale

        @pl.when(my_y == 0)
        def _():
            for i in range(1, len(EARLY_CHUNKS)):
                load(i, EARLY_CHUNKS[i]).start()
            pl.semaphore_signal(barrier, inc=1, device_id=peer,
                                device_id_type=MESH)
            for i in range(2):
                load(i, EARLY_CHUNKS[i]).wait()
                reduce_chunk(EARLY_CHUNKS[i])
            pl.semaphore_wait(barrier, 1)
            up_last().start()
            for i, msg in ((2, up_lo), (3, up_mid)):
                load(i, EARLY_CHUNKS[i]).wait()
                reduce_chunk(EARLY_CHUNKS[i])
                msg().start()

            down_raw().wait_recv()
            known_mid = part[:, mid] + _squash(
                _scatter_row_sums(rawbuf, 0, RAW, RAW0 % LANES))
            up_last().wait_send()
            up_lo().wait_send()
            up_mid().wait_send()
            down_head().wait_recv()
            out_ref[:, lo] = (part[:, lo] + recv[:, lo]) * scale
            out_ref[:, mid] = (known_mid + recv[:, mid]) * scale
            down_last().wait_recv()

    out = pl.pallas_call(
        body,
        out_shape=jax.ShapeDtypeStruct((1, m), jnp.float32),
        in_specs=[pl.BlockSpec(memory_space=pl.ANY)],
        out_specs=pl.BlockSpec(memory_space=pltpu.VMEM),
        scratch_shapes=[
            pltpu.VMEM((m, n), jnp.float32),
            pltpu.VMEM((RAW, n), jnp.float32),
            pltpu.VMEM((1, m), jnp.float32),
            pltpu.VMEM((1, m), jnp.float32),
            pltpu.SemaphoreType.DMA((len(LATE_CHUNKS),)),
            pltpu.SemaphoreType.DMA((3,)),
            pltpu.SemaphoreType.DMA((3,)),
        ],
        compiler_params=_compiler_params(),
    )(x)
    return out.reshape(m, 1)
```
